```python
import numpy as np

kernel_name = "dist_moe_shared_ep_outshard_n256_d128_e2_h256"

def setup_inputs():
    x = np.random.randn(256, 128).astype(np.float32)
    router_W = np.random.randn(128, 8).astype(np.float32) * 0.1
    scores64 = x.astype(np.float64) @ router_W.astype(np.float64)
    route_idx = np.argsort(-scores64, axis=-1)[:, :1].astype(np.int32)
    expert_W = np.random.randn(8, 128, 256).astype(np.float32) * 0.02
    shared_W = np.random.randn(128, 256).astype(np.float32) * 0.02
    return {"x": x, "router_W": router_W, "route_idx": route_idx, "expert_W": expert_W, "shared_W": shared_W}

def reference(x, router_W, route_idx, expert_W, shared_W):
    scores = x @ router_W
    s_max = scores.max(axis=-1, keepdims=True)
    probs = np.exp(scores - s_max)
    probs = probs / probs.sum(axis=-1, keepdims=True)
    shared = x @ shared_W
    out = np.zeros((256, 256), dtype=np.float32)
    for i in range(256):
        e = int(route_idx[i, 0])
        out[i] = shared[i] + probs[i, e] * (x[i] @ expert_W[e])
    return out
```

```python
import functools

import jax
import jax.numpy as jnp
from jax import lax
from jax.experimental import pallas as pl
from jax.experimental.pallas import tpu as pltpu

N_DEV = 4
N_TOK = 256
D_IN = 128
D_OUT = 256
N_EXP = 8
LOCAL_EXP = N_EXP // N_DEV
ROWS = N_TOK // N_DEV
LANES = 128
WORD = 32

MESH = pl.DeviceIdType.MESH
BF16, F32, I32, U32 = jnp.bfloat16, jnp.float32, jnp.int32, jnp.uint32


def _pack(y):
    bits = lax.bitcast_convert_type(y.astype(BF16).astype(F32), U32)
    return (bits[:, :LANES] >> 16) | bits[:, LANES:]


def _unpack(u):
    lo = lax.bitcast_convert_type(u << 16, F32)
    hi = lax.bitcast_convert_type(u & jnp.uint32(0xFFFF0000), F32)
    return lo, hi


def _routing_masks(route, block, first_expert):
    sub = lax.broadcasted_iota(I32, (8, LANES), 0)
    lane = lax.broadcasted_iota(I32, (8, LANES), 1)
    start = block * ROWS // LANES * LANES
    tokens = jnp.broadcast_to(route[:, start:start + LANES], (8, LANES))
    hit = (tokens == first_expert + (sub >> 2)) & (
        (lane >> 4) == (block * ROWS - start) // 16 + (sub & 3))
    bit = (1 << (15 - (lane & 15))).astype(F32)
    half = jnp.sum(jnp.where(hit, bit, 0.0), axis=1, keepdims=True).astype(I32)
    return [[(half[4 * j + 2 * h, 0] << 16) | half[4 * j + 2 * h + 1, 0]
             for h in range(ROWS // WORD)] for j in range(LOCAL_EXP)]


def _without_top_bit(mask, leading_zeros):
    return mask & lax.shift_right_logical(jnp.int32(2**31 - 1), leading_zeros & 31)


def _moe(x_hbm, router_hbm, route_hbm, expert_hbm, shared_hbm, out_ref,
         x_v, router_v, route_v, expert_v, shared_v, send_buf, recv_buf,
         load_sems, send_sem, recv_sem):
    head, tail = pl.ds(0, ROWS), pl.ds(ROWS, N_TOK - ROWS)
    load_route = pltpu.make_async_copy(route_hbm, route_v, load_sems.at[0])
    load_head = pltpu.make_async_copy(x_hbm.at[head], x_v.at[head], load_sems.at[1])
    load_tail = pltpu.make_async_copy(x_hbm.at[tail], x_v.at[tail], load_sems.at[2])
    load_router = pltpu.make_async_copy(router_hbm, router_v, load_sems.at[3])
    load_shared = pltpu.make_async_copy(shared_hbm, shared_v, load_sems.at[4])
    load_expert = [
        pltpu.make_async_copy(expert_hbm.at[j], expert_v.at[j], load_sems.at[5 + j])
        for j in range(LOCAL_EXP)]

    for load in (load_route, load_head, *load_expert):
        load.start()
    me = lax.axis_index("i")
    barrier = pltpu.get_barrier_semaphore()
    for k in (2, 1, 3):
        pl.semaphore_signal(barrier, inc=1, device_id=((me + k) & (N_DEV - 1),),
                            device_id_type=MESH)

    load_route.wait()
    for load in (load_tail, load_router, load_shared):
        load.start()
    route = route_v[...] & (N_EXP - 1)
    masks = [_routing_masks(route, block, LOCAL_EXP * me) for block in range(N_DEV)]

    def row_copy(block, j, row):
        return pltpu.make_async_remote_copy(
            src_ref=send_buf.at[j, pl.ds(block * ROWS + row, 1)],
            dst_ref=recv_buf.at[pl.ds(row, 1)],
            send_sem=send_sem, recv_sem=recv_sem,
            device_id=(block,), device_id_type=MESH)

    def send_all(block, j):
        for h, mask in enumerate(masks[block][j]):
            def step(mask, h=h):
                b = lax.clz(mask)
                row_copy(block, j, WORD * h + b).start()
                return _without_top_bit(mask, b)
            lax.while_loop(lambda mask: mask != 0, step, mask)

    def send_next(j, h, stored=WORD):
        mask = masks[0][j][h]
        b = lax.clz(mask)
        pl.when(b < stored)(lambda: row_copy(0, j, WORD * h + b).start())
        rest = _without_top_bit(mask, b)
        masks[0][j][h] = rest if stored == WORD else jnp.where(b < stored, rest, mask)

    def store_and_send(j, packed):
        for r in range(0, ROWS, 8):
            send_buf[j, pl.ds(r, 8), :] = packed[r:r + 8]
            send_next(j, 0, min(r + 8, WORD))

    def expert_rows(xb, j):
        return _pack(jnp.dot(xb, expert_v[j].astype(BF16), preferred_element_type=F32))

    pl.when(me != 0)(lambda: pl.semaphore_wait(barrier, N_DEV - 1))

    load_head.wait()
    xb = x_v[head, :].astype(BF16)
    load_expert[0].wait()
    store_and_send(0, expert_rows(xb, 0))
    load_expert[1].wait()
    packed = expert_rows(xb, 1)
    for _ in range(8):
        send_next(0, 1)
    store_and_send(1, packed)
    for _ in range(6):
        send_next(1, 1)
    for j in range(LOCAL_EXP):
        send_all(0, j)

    load_tail.wait()
    xb = x_v[tail, :].astype(BF16)
    for j in range(LOCAL_EXP):
        send_buf[j, tail, :] = expert_rows(xb, j)
    pl.when(me == 0)(lambda: pl.semaphore_wait(barrier, N_DEV - 1))
    for block in (1, 3, 2):
        for j in range(LOCAL_EXP):
            send_all(block, j)

    load_router.wait()
    load_shared.wait()
    scores = lax.dot_general(
        router_v[...], x_v[...], (((1,), (1,)), ((), ())),
        precision=lax.Precision.HIGHEST, preferred_element_type=F32)
    probs = jnp.exp(scores - jnp.max(scores, axis=0, keepdims=True))
    chosen = lax.broadcasted_iota(I32, probs.shape, 0) == route
    gate = (jnp.sum(jnp.where(chosen, probs, 0.0), axis=0, keepdims=True)
            / jnp.sum(probs, axis=0, keepdims=True))
    first = pl.multiple_of(me * ROWS, ROWS)
    mine = (lax.broadcasted_iota(I32, (ROWS, N_TOK), 1)
            == first + lax.broadcasted_iota(I32, (ROWS, N_TOK), 0))
    gate = jnp.sum(jnp.where(mine, gate, 0.0), axis=1, keepdims=True)
    shared = jnp.dot(x_v[pl.ds(first, ROWS), :].astype(BF16),
                     shared_v[...].astype(BF16), preferred_element_type=F32)

    n_sent = jnp.sum(jnp.where((route >> 1) == me, 1.0, 0.0),
                     axis=1, keepdims=True).astype(I32)[0, 0]
    for trips, per_trip in ((n_sent >> 3, 8), (n_sent & 7, 1)):
        @pl.loop(0, trips)
        def _(_, per_trip=per_trip):
            for _ in range(per_trip):
                row_copy(0, 0, 0).wait_send()

    pltpu.make_async_copy(recv_buf, recv_buf, recv_sem).wait()
    lo, hi = _unpack(recv_buf[...])
    out_ref[:, :LANES] = shared[:, :LANES] + gate * lo
    out_ref[:, LANES:] = shared[:, LANES:] + gate * hi


def _body(*refs):
    pl.run_scoped(
        functools.partial(_moe, *refs),
        pltpu.SemaphoreType.DMA((5 + LOCAL_EXP,)),
        pltpu.SemaphoreType.DMA,
        pltpu.SemaphoreType.DMA)


def pallas_dist_moe_shared_ep_outshard_n256_d128_e2_h256_kernel(
    x: jax.Array,
    router_W: jax.Array,
    route_idx: jax.Array,
    expert_W: jax.Array,
    shared_W: jax.Array,
):
    return pl.pallas_call(
        _body,
        out_shape=jax.ShapeDtypeStruct((ROWS, D_OUT), F32),
        in_specs=[pl.BlockSpec(memory_space=pltpu.HBM)] * 5,
        out_specs=pl.BlockSpec(memory_space=pltpu.VMEM),
        scratch_shapes=[
            pltpu.VMEM((N_TOK, D_IN), F32),
            pltpu.VMEM((N_EXP, D_IN), F32),
            pltpu.VMEM((1, N_TOK), I32),
            pltpu.VMEM((LOCAL_EXP, D_IN, D_OUT), F32),
            pltpu.VMEM((D_IN, D_OUT), F32),
            pltpu.VMEM((LOCAL_EXP, N_TOK, LANES), U32),
            pltpu.VMEM((ROWS, LANES), U32),
        ],
        compiler_params=pltpu.CompilerParams(collective_id=0),
    )(x, router_W.T, route_idx.reshape(1, N_TOK), expert_W, shared_W)
```
